```python
import numpy as np

kernel_name = "dist_moe_shared_ep_outshard_n256_d128_e2_h256"

def setup_inputs():
    x = np.random.randn(256, 128).astype(np.float32)
    router_W = np.random.randn(128, 8).astype(np.float32) * 0.1
    scores64 = x.astype(np.float64) @ router_W.astype(np.float64)
    route_idx = np.argsort(-scores64, axis=-1)[:, :1].astype(np.int32)
    expert_W = np.random.randn(8, 128, 256).astype(np.float32) * 0.02
    shared_W = np.random.randn(128, 256).astype(np.float32) * 0.02
    return {"x": x, "router_W": router_W, "route_idx": route_idx, "expert_W": expert_W, "shared_W": shared_W}

def reference(x, router_W, route_idx, expert_W, shared_W):
    scores = x @ router_W
    s_max = scores.max(axis=-1, keepdims=True)
    probs = np.exp(scores - s_max)
    probs = probs / probs.sum(axis=-1, keepdims=True)
    shared = x @ shared_W
    out = np.zeros((256, 256), dtype=np.float32)
    for i in range(256):
        e = int(route_idx[i, 0])
        out[i] = shared[i] + probs[i, e] * (x[i] @ expert_W[e])
    return out
```

```python
import jax, jax.numpy as jnp
from jax import lax
from jax.experimental import pallas as pl
from jax.experimental.pallas import tpu as pltpu

N_DEV, TOK, D, H = 4, 64, 128, 256
BF = jnp.bfloat16
F32 = jnp.float32

def body(x_hbm, rw_hbm, r_hbm, w_hbm, s_hbm, o_ref, xv, rwv, rv, wv, sv, rcol, sbuf, rbuf, lsem, ssem, rsem):
    me = lax.axis_index("i")
    order = (2, 1, 3)
    peers = [lax.rem(me + k, N_DEV) for k in order]
    cp_r = pltpu.make_async_copy(r_hbm, rv, lsem.at[0])
    cp_x = pltpu.make_async_copy(x_hbm, xv, lsem.at[1])
    cp_w = pltpu.make_async_copy(w_hbm, wv, lsem.at[2])
    cp_rw = pltpu.make_async_copy(rw_hbm, rwv, lsem.at[3])
    cp_s = pltpu.make_async_copy(s_hbm, sv, lsem.at[4])
    cp_r.start(); cp_x.start(); cp_w.start()
    bar = pltpu.get_barrier_semaphore()
    for p in peers:
        pl.semaphore_signal(bar, inc=1, device_id=(p,), device_id_type=pl.DeviceIdType.MESH)
    cp_r.wait()
    for h in range(2):
        row = rv[:, 128 * h:128 * (h + 1)]
        rcol[128 * h:128 * (h + 1), :] = jnp.broadcast_to(row, (128, 128)).T
    cp_x.wait()
    cp_w.wait()
    cp_rw.start(); cp_s.start()
    w = wv[...].reshape(2 * D, H).astype(BF)

    def partial(blk):
        rows = pl.ds(pl.multiple_of(blk * TOK, TOK), TOK)
        xb = xv[rows, :]
        rb = rcol[rows, :]
        lhs = jnp.concatenate([jnp.where(rb == 2 * me, xb, 0.0), jnp.where(rb == 2 * me + 1, xb, 0.0)], axis=1).astype(BF)
        return jnp.dot(lhs, w, preferred_element_type=F32)

    rdmas = []
    for j, p in enumerate(peers):
        sbuf[j] = partial(p).astype(BF)
        if j == 0:
            pl.semaphore_wait(bar, 3)
        c = pltpu.make_async_remote_copy(sbuf.at[j], rbuf.at[j], ssem.at[j], rsem.at[j], device_id=(p,), device_id_type=pl.DeviceIdType.MESH)
        c.start()
        rdmas.append(c)
    own = partial(me)
    rows = pl.ds(pl.multiple_of(me * TOK, TOK), TOK)
    xm = xv[rows, :]
    cp_rw.wait()
    sc = lax.dot_general(xm, rwv[...], (((1,), (1,)), ((), ())), preferred_element_type=F32, precision=lax.Precision.HIGHEST)
    ex = jnp.exp(sc - jnp.max(sc, axis=-1, keepdims=True))
    sel = lax.broadcasted_iota(jnp.int32, (TOK, 8), 1) == rcol[rows, 0:8]
    g = jnp.sum(jnp.where(sel, ex, 0.0), axis=-1, keepdims=True) / jnp.sum(ex, axis=-1, keepdims=True)
    cp_s.wait()
    acc = jnp.dot(xm.astype(BF), sv[...].astype(BF), preferred_element_type=F32) + g * own
    o_ref[...] = acc
    for j in (1, 2, 0):
        rdmas[j].wait_recv()
        o_ref[...] += g * rbuf[j].astype(F32)
    for c in rdmas:
        c.wait_send()

def pallas_dist_moe_shared_ep_outshard_n256_d128_e2_h256_kernel(x, router_W, route_idx, expert_W, shared_W):
    return pl.pallas_call(
        body,
        out_shape=jax.ShapeDtypeStruct((TOK, H), F32),
        in_specs=[pl.BlockSpec(memory_space=pltpu.HBM)] * 5,
        out_specs=pl.BlockSpec(memory_space=pltpu.VMEM),
        scratch_shapes=[
            pltpu.VMEM((N_DEV * TOK, D), F32), pltpu.VMEM((8, D), F32), pltpu.VMEM((1, 256), jnp.int32),
            pltpu.VMEM((2, D, H), F32), pltpu.VMEM((D, H), F32), pltpu.VMEM((256, 128), jnp.int32),
            pltpu.VMEM((3, TOK, H), BF), pltpu.VMEM((3, TOK, H), BF),
            pltpu.SemaphoreType.DMA((5,)), pltpu.SemaphoreType.DMA((3,)), pltpu.SemaphoreType.DMA((3,)),
        ],
        compiler_params=pltpu.CompilerParams(collective_id=0, disable_bounds_checks=True, disable_semaphore_checks=True),
        name="kern",
    )(x, router_W.T, route_idx.reshape(1, 256), expert_W, shared_W)
```

```python
import jax
import jax.numpy as jnp
from jax import lax
from jax.experimental import pallas as pl
from jax.experimental.pallas import tpu as pltpu

N_DEV, N_EXP, TOK, D, H, LANES = 4, 8, 64, 128, 256, 128
SIZES = (16, 24, 32)
CAP = SIZES[-1]
FAR, NEAR = 2, (1, 3)
BF16, F32, I32 = jnp.bfloat16, jnp.float32, jnp.int32


def _iota(shape, dim):
    return lax.broadcasted_iota(I32, shape, dim)


def _take_rows(table, idx):
    dims = lax.GatherDimensionNumbers(
        offset_dims=(),
        collapsed_slice_dims=(0,),
        start_index_map=(0,),
        operand_batching_dims=(1,),
        start_indices_batching_dims=(1,),
    )
    return lax.gather(table, idx.reshape(*idx.shape, 1), dims, (1, 1),
                      mode=lax.GatherScatterMode.PROMISE_IN_BOUNDS)


def _mm(a, b):
    return jnp.dot(a.astype(BF16), b.astype(BF16), preferred_element_type=F32)


def _sized(count, fn):
    small, medium, large = SIZES
    pl.when(count <= small)(lambda: fn(small))
    pl.when((count > small) & (count <= medium))(lambda: fn(medium))
    pl.when(count > medium)(lambda: fn(large))


def _for_each_overflow(count, fn):
    @pl.when(jnp.maximum(jnp.maximum(count[1], count[2]), count[3]) > CAP)
    def _():
        @pl.loop(1, N_DEV)
        def _(k):
            n = jnp.where(k == 1, count[1], jnp.where(k == 2, count[2], count[3]))
            pl.when(n > CAP)(lambda: fn(k))


def _body(x_hbm, router_hbm, route_hbm, w_hbm, shared_hbm, out_ref,
          x_v, router_v, route_v, w_v, shared_v,
          far_out, far_in, near_out, near_in, full_out, full_in,
          load_sem, send_sem, recv_sem, full_send_sem, full_recv_sem):
    me = lax.axis_index("i")
    halves = [pl.ds(LANES * h, LANES) for h in range(2)]

    def x_copy(k, sem):
        rows = pl.ds(pl.multiple_of((me ^ k) * TOK, TOK), TOK)
        return pltpu.make_async_copy(x_hbm.at[rows], x_v.at[k], sem)

    def remote(src, dst, s_sem, r_sem, k):
        return pltpu.make_async_remote_copy(
            src, dst, s_sem, r_sem,
            device_id=(me ^ k,), device_id_type=pl.DeviceIdType.MESH)

    def far(h, rows):
        return remote(far_out.at[h, pl.ds(0, rows)], far_in.at[h, pl.ds(0, rows)],
                      send_sem.at[h], recv_sem.at[h], FAR)

    def near(j, rows):
        return remote(near_out.at[j, pl.ds(0, rows)], near_in.at[j, pl.ds(0, rows)],
                      send_sem.at[2 + j], recv_sem.at[2 + j], NEAR[j])

    def full(k):
        return remote(full_out, full_in.at[k - 1], full_send_sem, full_recv_sem.at[k - 1], k)

    def experts(h):
        return w_v[h].reshape(2 * D, LANES)

    ld_route = pltpu.make_async_copy(route_hbm, route_v, load_sem.at[0])
    ld_far = x_copy(FAR, load_sem.at[1])
    ld_w = [pltpu.make_async_copy(w_hbm.at[:, :, halves[h]], w_v.at[h], load_sem.at[2 + h])
            for h in range(2)]
    ld_near = [x_copy(k, load_sem.at[4]) for k in NEAR]
    ld_own = [x_copy(0, load_sem.at[5]),
              pltpu.make_async_copy(router_hbm, router_v, load_sem.at[5])]
    ld_shared = pltpu.make_async_copy(shared_hbm, shared_v, load_sem.at[6])
    for ld in (ld_route, ld_far, *ld_w):
        ld.start()
    far_in[:, SIZES[0]:, :] = jnp.zeros((2, CAP - SIZES[0], LANES), BF16)
    near_in[:, SIZES[0]:, :] = jnp.zeros((2, CAP - SIZES[0], H), BF16)
    barrier = pltpu.get_barrier_semaphore()
    for k in (FAR, *NEAR):
        pl.semaphore_signal(barrier, inc=1, device_id=(me ^ k,),
                            device_id_type=pl.DeviceIdType.MESH)

    suffix = jnp.where(_iota((LANES, LANES), 0) >= _iota((LANES, LANES), 1), 1.0, 0.0)
    odd = ((_iota((8, LANES), 1) >> 6) ^ me) & 1
    ld_route.wait()
    raw = [jnp.broadcast_to(route_v[:, halves[h]], (8, LANES)) & (N_EXP - 1) for h in range(2)]
    route = [jnp.where(me >= 2, raw[1 - t], raw[t]) for t in range(2)]
    rel = [r ^ (2 * me) for r in route]
    group = [4 * odd + (r >> 1) for r in rel]
    member = jnp.concatenate(
        [jnp.where(g == _iota((8, LANES), 0), 1.0, 0.0) for g in group], axis=0)
    seen = _mm(member, suffix)
    ld_far.wait()
    seen = seen.astype(I32)
    seen = [seen[:8], seen[8:]]
    code = [(N_EXP * odd + rel[t]) * TOK + _take_rows(seen[t], group[t]) - 1 for t in range(2)]
    n_out = {k: seen[k >> 1][4 * (k & 1), 0] for k in (FAR, *NEAR)}
    n_in = {k: seen[0][k, 0] for k in (*NEAR, FAR)}

    def pack(k):
        c = jnp.concatenate([code[k >> 1]] * (CAP // 8), axis=0)
        xb = x_v[k]
        xb = jnp.concatenate([xb, xb], axis=0)
        first = [(N_EXP * (k & 1) + e) * TOK for e in range(2)]
        return jnp.concatenate(
            [_mm(jnp.where(c == f + _iota((CAP, LANES), 0), 1.0, 0.0), xb) for f in first],
            axis=1)

    packed = pack(FAR)
    for h in range(2):
        ld_w[h].wait()
        if h == 0:
            for ld in (*ld_near, *ld_own, ld_shared):
                ld.start()
        w = experts(h)
        for r in (slice(0, CAP // 2), slice(CAP // 2, CAP)):
            far_out[h, r, :] = _mm(packed[r], w).astype(BF16)
        if h == 0:
            pl.semaphore_wait(barrier, N_DEV - 1)
        _sized(n_out[FAR], lambda rows: far(h, rows).start())

    for ld in ld_near:
        ld.wait()
    packed = jnp.concatenate([pack(k) for k in NEAR], axis=0)
    y = jnp.concatenate([_mm(packed, experts(h)) for h in range(2)], axis=1).astype(BF16)
    for j, k in enumerate(NEAR):
        near_out[j] = y[CAP * j:CAP * (j + 1)]
        _sized(n_out[k], lambda rows: near(j, rows).start())

    def to_rows(lanes, k):
        t = jnp.concatenate([lanes] * (LANES // 8), axis=0).T
        return jnp.where(((me ^ k) & 1) == 1, t[TOK:], t[:TOK])

    def unpacked(xb, e):
        lhs = jnp.concatenate([jnp.where(e == 0, xb, 0.0), jnp.where(e == 1, xb, 0.0)], axis=1)
        return jnp.concatenate([_mm(lhs, experts(h)) for h in range(2)], axis=1)

    def send_full(k):
        e = to_rows(jnp.where(k >= 2, rel[1], rel[0]), k)
        full_out[...] = unpacked(x_v[k], e).astype(BF16)
        copy = full(k)
        copy.start()
        copy.wait_send()

    _for_each_overflow(n_out, send_full)

    for ld in ld_own:
        ld.wait()
    x_own = x_v[0]
    scores = lax.dot_general(
        router_v[...], jnp.concatenate([x_own, x_own], axis=0), (((1,), (1,)), ((), ())),
        precision=lax.Precision.HIGHEST, preferred_element_type=F32)
    ex = jnp.exp(scores - jnp.max(scores, axis=0, keepdims=True))
    gate = to_rows(_take_rows(ex, route[0]) / jnp.sum(ex, axis=0, keepdims=True), 0)
    own = to_rows(code[0], 0)
    source, slot = own >> 7, own & (TOK - 1)
    ld_shared.wait()
    out_ref[...] = (_mm(x_own, shared_v[...])
                    + jnp.concatenate([gate, gate], axis=1) * unpacked(x_own, own >> 6))

    def add_full(k):
        full(k).wait_recv()
        g = jnp.where((source == k) & (slot >= CAP), gate, 0.0)
        out_ref[...] += jnp.concatenate([g, g], axis=1) * full_in[k - 1].astype(F32)

    _for_each_overflow(n_in, add_full)

    low, bit3, bit4 = slot & 7, (slot & 8) != 0, (slot & 16) != 0

    def add_packed(y, g, h):
        y = y.astype(F32)
        rows = []
        for t in range(TOK // 8):
            r = slice(8 * t, 8 * t + 8)
            v = [_take_rows(y[8 * q:8 * q + 8], low[r]) for q in range(CAP // 8)]
            rows.append(g[r] * jnp.where(bit4[r],
                                         jnp.where(bit3[r], v[3], v[2]),
                                         jnp.where(bit3[r], v[1], v[0])))
        out_ref[:, halves[h]] += jnp.concatenate(rows, axis=0)

    def gate_of(k):
        return jnp.where((source == k) & (slot < CAP), gate, 0.0)

    for i in range(2):
        _sized(n_out[FAR], lambda rows: far(i, rows).wait_send())
        _sized(n_out[NEAR[i]], lambda rows: near(i, rows).wait_send())
    for j in (1, 0):
        g = gate_of(NEAR[j])
        _sized(n_in[NEAR[j]], lambda rows: near(j, rows).wait_recv())
        for h in range(2):
            add_packed(near_in[j, :, halves[h]], g, h)
    g = gate_of(FAR)
    for h in range(2):
        _sized(n_in[FAR], lambda rows: far(h, rows).wait_recv())
        add_packed(far_in[h], g, h)


def pallas_dist_moe_shared_ep_outshard_n256_d128_e2_h256_kernel(
    x: jax.Array,
    router_W: jax.Array,
    route_idx: jax.Array,
    expert_W: jax.Array,
    shared_W: jax.Array,
):
    return pl.pallas_call(
        _body,
        out_shape=jax.ShapeDtypeStruct((TOK, H), F32),
        in_specs=[pl.BlockSpec(memory_space=pltpu.HBM)] * 5,
        out_specs=pl.BlockSpec(memory_space=pltpu.VMEM),
        scratch_shapes=[
            pltpu.VMEM((N_DEV, TOK, D), F32),
            pltpu.VMEM((N_EXP, D), F32),
            pltpu.VMEM((1, N_DEV * TOK), I32),
            pltpu.VMEM((2, 2, D, LANES), F32),
            pltpu.VMEM((D, H), F32),
            pltpu.VMEM((2, CAP, LANES), BF16),
            pltpu.VMEM((2, CAP, LANES), BF16),
            pltpu.VMEM((2, CAP, H), BF16),
            pltpu.VMEM((2, CAP, H), BF16),
            pltpu.VMEM((TOK, H), BF16),
            pltpu.VMEM((N_DEV - 1, TOK, H), BF16),
            pltpu.SemaphoreType.DMA((7,)),
            pltpu.SemaphoreType.DMA((4,)),
            pltpu.SemaphoreType.DMA((4,)),
            pltpu.SemaphoreType.DMA,
            pltpu.SemaphoreType.DMA((N_DEV - 1,)),
        ],
        compiler_params=pltpu.CompilerParams(collective_id=0, disable_semaphore_checks=True),
    )(x, router_W.T, route_idx.reshape(1, N_DEV * TOK), expert_W, shared_W)
```

```python
import functools

import jax
import jax.numpy as jnp
from jax import lax
from jax.experimental import pallas as pl
from jax.experimental.pallas import tpu as pltpu

N_DEV, N_EXP, TOK, D, H, LANES = 4, 8, 64, 128, 256, 128
SIZES = (16, 24, 32)
CAP = SIZES[-1]
FAR, NEAR = 2, (1, 3)
BF16, F32, I32 = jnp.bfloat16, jnp.float32, jnp.int32


def _iota(shape, dim):
    return lax.broadcasted_iota(I32, shape, dim)


def _take_rows(table, idx):
    dims = lax.GatherDimensionNumbers(
        offset_dims=(),
        collapsed_slice_dims=(0,),
        start_index_map=(0,),
        operand_batching_dims=(1,),
        start_indices_batching_dims=(1,),
    )
    return lax.gather(table, idx.reshape(*idx.shape, 1), dims, (1, 1),
                      mode=lax.GatherScatterMode.PROMISE_IN_BOUNDS)


def _mm(a, b):
    return jnp.dot(a.astype(BF16), b.astype(BF16), preferred_element_type=F32)


def _sized(count, fn):
    small, medium, large = SIZES
    pl.when(count <= small)(lambda: fn(small))
    pl.when((count > small) & (count <= medium))(lambda: fn(medium))
    pl.when(count > medium)(lambda: fn(large))


def _for_each_overflow(count, fn):
    @pl.when(jnp.maximum(jnp.maximum(count[1], count[2]), count[3]) > CAP)
    def _():
        @pl.loop(1, N_DEV)
        def _(k):
            n = jnp.where(k == 1, count[1], jnp.where(k == 2, count[2], count[3]))
            pl.when(n > CAP)(lambda: fn(k))


def _body(x_hbm, router_hbm, route_hbm, w_hbm, shared_hbm, out_ref,
          x_v, router_v, route_v, w_v, shared_v,
          far_out, far_in, near_out, near_in, full_out, full_in,
          load_sem, send_sem, recv_sem, full_send_sem, full_recv_sem):
    me = lax.axis_index("i")
    halves = [pl.ds(LANES * h, LANES) for h in range(2)]

    def x_copy(k, sem):
        rows = pl.ds(pl.multiple_of((me ^ k) * TOK, TOK), TOK)
        return pltpu.make_async_copy(x_hbm.at[rows], x_v.at[k], sem)

    def remote(src, dst, s_sem, r_sem, k):
        return pltpu.make_async_remote_copy(
            src, dst, s_sem, r_sem,
            device_id=(me ^ k,), device_id_type=pl.DeviceIdType.MESH)

    def far(h, rows):
        return remote(far_out.at[h, pl.ds(0, rows)], far_in.at[h, pl.ds(0, rows)],
                      send_sem.at[h], recv_sem.at[h], FAR)

    def near(j, rows):
        return remote(near_out.at[j, pl.ds(0, rows)], near_in.at[j, pl.ds(0, rows)],
                      send_sem.at[2 + j], recv_sem.at[2 + j], NEAR[j])

    def full(k):
        return remote(full_out, full_in.at[k - 1], full_send_sem, full_recv_sem.at[k - 1], k)

    def experts(h):
        return w_v[h].reshape(2 * D, LANES)

    ld_route = pltpu.make_async_copy(route_hbm, route_v, load_sem.at[0])
    ld_far = x_copy(FAR, load_sem.at[1])
    ld_w = [pltpu.make_async_copy(w_hbm.at[:, :, halves[h]], w_v.at[h], load_sem.at[2 + h])
            for h in range(2)]
    ld_near = [x_copy(k, load_sem.at[4]) for k in NEAR]
    ld_own = [x_copy(0, load_sem.at[5]),
              pltpu.make_async_copy(router_hbm, router_v, load_sem.at[5])]
    ld_shared = pltpu.make_async_copy(shared_hbm, shared_v, load_sem.at[6])
    for ld in (ld_route, ld_far, *ld_w):
        ld.start()
    far_in[:, SIZES[0]:, :] = jnp.zeros((2, CAP - SIZES[0], LANES), BF16)
    near_in[:, SIZES[0]:, :] = jnp.zeros((2, CAP - SIZES[0], H), BF16)
    barrier = pltpu.get_barrier_semaphore()
    for k in (FAR, *NEAR):
        pl.semaphore_signal(barrier, inc=1, device_id=(me ^ k,),
                            device_id_type=pl.DeviceIdType.MESH)

    suffix = jnp.where(_iota((LANES, LANES), 0) >= _iota((LANES, LANES), 1), 1.0, 0.0)
    odd = ((_iota((8, LANES), 1) >> 6) ^ me) & 1
    ld_route.wait()
    raw = [jnp.broadcast_to(route_v[:, halves[h]], (8, LANES)) & (N_EXP - 1) for h in range(2)]
    route = [jnp.where(me >= 2, raw[1 - t], raw[t]) for t in range(2)]
    rel = [r ^ (2 * me) for r in route]
    group = [4 * odd + (r >> 1) for r in rel]
    member = jnp.concatenate(
        [jnp.where(g == _iota((8, LANES), 0), 1.0, 0.0) for g in group], axis=0)
    seen = _mm(member, suffix)
    ld_far.wait()
    seen = seen.astype(I32)
    seen = [seen[:8], seen[8:]]
    code = [(N_EXP * odd + rel[t]) * TOK + _take_rows(seen[t], group[t]) - 1 for t in range(2)]
    n_out = {k: seen[k >> 1][4 * (k & 1), 0] for k in (FAR, *NEAR)}
    n_in = {k: seen[0][k, 0] for k in (*NEAR, FAR)}

    def pack(k):
        c = jnp.concatenate([code[k >> 1]] * (CAP // 8), axis=0)
        xb = x_v[k]
        xb = jnp.concatenate([xb, xb], axis=0)
        first = [(N_EXP * (k & 1) + e) * TOK for e in range(2)]
        return jnp.concatenate(
            [_mm(jnp.where(c == f + _iota((CAP, LANES), 0), 1.0, 0.0), xb) for f in first],
            axis=1)

    packed = pack(FAR)
    for h in range(2):
        ld_w[h].wait()
        if h == 0:
            for ld in (*ld_near, *ld_own, ld_shared):
                ld.start()
        w = experts(h)
        for r in (slice(0, CAP // 2), slice(CAP // 2, CAP)):
            far_out[h, r, :] = _mm(packed[r], w).astype(BF16)
        if h == 0:
            pl.semaphore_wait(barrier, N_DEV - 1)
        _sized(n_out[FAR], lambda rows: far(h, rows).start())

    for ld in ld_near:
        ld.wait()
    packed = jnp.concatenate([pack(k) for k in NEAR], axis=0)
    y = jnp.concatenate([_mm(packed, experts(h)) for h in range(2)], axis=1).astype(BF16)
    for j, k in enumerate(NEAR):
        near_out[j] = y[CAP * j:CAP * (j + 1)]
        _sized(n_out[k], lambda rows: near(j, rows).start())

    def to_rows(lanes, k):
        t = jnp.concatenate([lanes] * (LANES // 8), axis=0).T
        return jnp.where(((me ^ k) & 1) == 1, t[TOK:], t[:TOK])

    def unpacked(xb, e):
        lhs = jnp.concatenate([jnp.where(e == 0, xb, 0.0), jnp.where(e == 1, xb, 0.0)], axis=1)
        return jnp.concatenate([_mm(lhs, experts(h)) for h in range(2)], axis=1)

    def send_full(k):
        e = to_rows(jnp.where(k >= 2, rel[1], rel[0]), k)
        full_out[...] = unpacked(x_v[k], e).astype(BF16)
        copy = full(k)
        copy.start()
        copy.wait_send()

    _for_each_overflow(n_out, send_full)

    for ld in ld_own:
        ld.wait()
    x_own = x_v[0]
    scores = lax.dot_general(
        router_v[...], jnp.concatenate([x_own, x_own], axis=0), (((1,), (1,)), ((), ())),
        precision=lax.Precision.HIGHEST, preferred_element_type=F32)
    ex = jnp.exp(scores - jnp.max(scores, axis=0, keepdims=True))
    gate = to_rows(_take_rows(ex, route[0]) / jnp.sum(ex, axis=0, keepdims=True), 0)
    own = to_rows(code[0], 0)
    source, slot = own >> 7, own & (TOK - 1)
    ld_shared.wait()
    out_ref[...] = (_mm(x_own, shared_v[...])
                    + jnp.concatenate([gate, gate], axis=1) * unpacked(x_own, own >> 6))

    def add_full(k):
        full(k).wait_recv()
        g = jnp.where((source == k) & (slot >= CAP), gate, 0.0)
        out_ref[...] += jnp.concatenate([g, g], axis=1) * full_in[k - 1].astype(F32)

    _for_each_overflow(n_in, add_full)

    low, bit3, bit4 = slot & 7, (slot & 8) != 0, (slot & 16) != 0

    def add_packed(y, g, h):
        y = y.astype(F32)
        rows = []
        for t in range(TOK // 8):
            r = slice(8 * t, 8 * t + 8)
            v = [_take_rows(y[8 * q:8 * q + 8], low[r]) for q in range(CAP // 8)]
            rows.append(g[r] * jnp.where(bit4[r],
                                         jnp.where(bit3[r], v[3], v[2]),
                                         jnp.where(bit3[r], v[1], v[0])))
        out_ref[:, halves[h]] += jnp.concatenate(rows, axis=0)

    def gate_of(k):
        return jnp.where((source == k) & (slot < CAP), gate, 0.0)

    for i in range(2):
        _sized(n_out[FAR], lambda rows: far(i, rows).wait_send())
        _sized(n_out[NEAR[i]], lambda rows: near(i, rows).wait_send())
    for j in (1, 0):
        g = gate_of(NEAR[j])
        _sized(n_in[NEAR[j]], lambda rows: near(j, rows).wait_recv())
        for h in range(2):
            add_packed(near_in[j, :, halves[h]], g, h)
    g = gate_of(FAR)
    for h in range(2):
        _sized(n_in[FAR], lambda rows: far(h, rows).wait_recv())
        add_packed(far_in[h], g, h)


def _kernel(*refs):
    pl.run_scoped(
        functools.partial(_body, *refs),
        pltpu.SemaphoreType.DMA((7,)),
        pltpu.SemaphoreType.DMA((4,)),
        pltpu.SemaphoreType.DMA((4,)),
        pltpu.SemaphoreType.DMA,
        pltpu.SemaphoreType.DMA((N_DEV - 1,)),
    )


def pallas_dist_moe_shared_ep_outshard_n256_d128_e2_h256_kernel(
    x: jax.Array,
    router_W: jax.Array,
    route_idx: jax.Array,
    expert_W: jax.Array,
    shared_W: jax.Array,
):
    return pl.pallas_call(
        _kernel,
        out_shape=jax.ShapeDtypeStruct((TOK, H), F32),
        in_specs=[pl.BlockSpec(memory_space=pltpu.HBM)] * 5,
        out_specs=pl.BlockSpec(memory_space=pltpu.VMEM),
        scratch_shapes=[
            pltpu.VMEM((N_DEV, TOK, D), F32),
            pltpu.VMEM((N_EXP, D), F32),
            pltpu.VMEM((1, N_DEV * TOK), I32),
            pltpu.VMEM((2, 2, D, LANES), F32),
            pltpu.VMEM((D, H), F32),
            pltpu.VMEM((2, CAP, LANES), BF16),
            pltpu.VMEM((2, CAP, LANES), BF16),
            pltpu.VMEM((2, CAP, H), BF16),
            pltpu.VMEM((2, CAP, H), BF16),
            pltpu.VMEM((TOK, H), BF16),
            pltpu.VMEM((N_DEV - 1, TOK, H), BF16),
        ],
        compiler_params=pltpu.CompilerParams(collective_id=0),
    )(x, router_W.T, route_idx.reshape(1, N_DEV * TOK), expert_W, shared_W)
```
